```python
import numpy as np

kernel_name = "dist_rmsnorm_colshard_i_m768_n512"

def setup_inputs():
    x = np.random.randn(768, 2048).astype(np.float32)
    gamma = np.random.randn(2048).astype(np.float32)
    return {"x": x, "gamma": gamma}

def reference(x: np.ndarray, gamma: np.ndarray) -> np.ndarray:
    eps = 1e-5
    rms = np.sqrt(np.mean(x * x, axis=1, keepdims=True) + eps)
    return gamma * x / rms
```

```python
import os
import jax
import jax.numpy as jnp
from jax import lax
from jax.experimental import pallas as pl
from jax.experimental.pallas import tpu as pltpu

N_DEV = 4
EPS = 1e-5
CHUNKS = tuple(int(c) for c in os.environ.get("CHUNKS", "320,256,128,64").split(","))
PEER_OFFS = (2, 1, 3)


def pallas_dist_rmsnorm_colshard_i_m768_n512_kernel(x, gamma):
    m, n = x.shape
    n_global = n * N_DEV
    assert sum(CHUNKS) == m
    nc = len(CHUNKS)
    starts = [sum(CHUNKS[:c]) for c in range(nc)]

    def body(x_hbm, g_hbm, out_ref, xbuf, gbuf, comm_ref, in_sems, g_sem, send_sems, recv_sems):
        my = lax.axis_index("i")
        in_cps = []
        for c in range(nc):
            cp = pltpu.make_async_copy(x_hbm.at[pl.ds(starts[c], CHUNKS[c])],
                                       xbuf.at[pl.ds(starts[c], CHUNKS[c])], in_sems.at[c])
            cp.start()
            in_cps.append(cp)
        g_cp = pltpu.make_async_copy(g_hbm, gbuf, g_sem)
        g_cp.start()

        barrier = pltpu.get_barrier_semaphore()
        for d in PEER_OFFS:
            pl.semaphore_signal(barrier, inc=1, device_id=((my + d) % N_DEV,),
                                device_id_type=pl.DeviceIdType.MESH)

        rdmas = []
        for c in range(nc):
            R = CHUNKS[c]
            G = R // 8
            in_cps[c].wait()
            xv = xbuf[pl.ds(starts[c], R), :]
            sq = xv * xv
            p = sq[:, 0:128]
            for j in range(1, n // 128):
                p = p + sq[:, j * 128:(j + 1) * 128]
            s = jnp.sum(p, axis=1, keepdims=True)
            s3 = jnp.broadcast_to(s, (R, 128)).reshape(G, 8, 128)
            lane = lax.broadcasted_iota(jnp.int32, (G, 8, 128), 2)
            grp = lax.broadcasted_iota(jnp.int32, (G, 8, 128), 0)
            packed = jnp.sum(jnp.where(lane == grp, s3, 0.0), axis=0)
            comm_ref[c, 0] = packed
            if c == 0:
                pl.semaphore_wait(barrier, N_DEV - 1)
            for k, d in enumerate(PEER_OFFS):
                r = pltpu.make_async_remote_copy(
                    src_ref=comm_ref.at[c, 0], dst_ref=comm_ref.at[c, d],
                    send_sem=send_sems.at[c * 3 + k], recv_sem=recv_sems.at[c * 3 + k],
                    device_id=((my + d) % N_DEV,), device_id_type=pl.DeviceIdType.MESH)
                r.start()
                rdmas.append(r)

        g_cp.wait()
        gv = gbuf[...]
        for c in range(nc):
            R = CHUNKS[c]
            G = R // 8
            for k in (1, 2, 0):
                rdmas[c * 3 + k].wait_recv()
            tot = (comm_ref[c, 0] + comm_ref[c, 1]) + (comm_ref[c, 3] + comm_ref[c, 2])
            rs = lax.rsqrt(tot * (1.0 / n_global) + EPS)
            for g in range(G):
                r0 = starts[c] + g * 8
                out_ref[pl.ds(r0, 8), :] = xbuf[pl.ds(r0, 8), :] * rs[:, g:g + 1] * gv
        for r in rdmas:
            r.wait_send()

    return pl.pallas_call(
        body,
        out_shape=jax.ShapeDtypeStruct((m, n), x.dtype),
        in_specs=[pl.BlockSpec(memory_space=pl.ANY), pl.BlockSpec(memory_space=pl.ANY)],
        out_specs=pl.BlockSpec(memory_space=pltpu.VMEM),
        scratch_shapes=[
            pltpu.VMEM((m, n), jnp.float32),
            pltpu.VMEM((1, n), jnp.float32),
            pltpu.VMEM((nc, N_DEV, 8, 128), jnp.float32),
            pltpu.SemaphoreType.DMA((nc,)),
            pltpu.SemaphoreType.DMA,
            pltpu.SemaphoreType.DMA((nc * 3,)),
            pltpu.SemaphoreType.DMA((nc * 3,)),
        ],
        compiler_params=pltpu.CompilerParams(collective_id=0),
    )(x, gamma.reshape(1, n))
```

```python
import math

import jax
import jax.numpy as jnp
from jax import lax
from jax.experimental import pallas as pl
from jax.experimental.pallas import tpu as pltpu

_N_DEV = 4
_EPS = 1e-5
_LANES = 128
_SUBLANES = 8
_GROUPS_PER_MSG_ROW = _LANES // _SUBLANES


def _row_chunks(m):
    if m == 768:
        return (256, 256, 128, 64, 64)
    assert m % _SUBLANES == 0
    chunks, left = [], m
    while left > 0:
        c = min(256, left)
        chunks.append(c)
        left -= c
    return tuple(chunks)


def pallas_dist_rmsnorm_colshard_i_m768_n512_kernel(x: jax.Array, gamma: jax.Array):
    m, n = x.shape
    assert n % _LANES == 0
    n_global = n * _N_DEV
    chunks = _row_chunks(m)
    nc = len(chunks)
    starts = [sum(chunks[:c]) for c in range(nc)]
    msg_rows = [-(-r // _LANES) for r in chunks]
    max_msg_rows = max(msg_rows)
    tile = (_SUBLANES, _LANES)

    def tree_sum(terms):
        while len(terms) > 1:
            nxt = [terms[i] + terms[i + 1] for i in range(0, len(terms) - 1, 2)]
            if len(terms) % 2:
                nxt.append(terms[-1])
            terms = nxt
        return terms[0]

    def body(x_hbm, g_hbm, out_ref,
             xbuf, gbuf, base_ref, send_ref, near_ref, diag_ref,
             in_sems, g_sem, send_sems, recv_sems):
        my = lax.axis_index("i")

        in_copies = []
        for c in range(nc):
            rows = pl.ds(starts[c], chunks[c])
            cp = pltpu.make_async_copy(x_hbm.at[rows], xbuf.at[rows], in_sems.at[c])
            cp.start()
            in_copies.append(cp)
        g_copy = pltpu.make_async_copy(g_hbm, gbuf, g_sem)
        g_copy.start()

        peers = [(my + 2) % _N_DEV, (my + 1) % _N_DEV, (my + 3) % _N_DEV]
        barrier = pltpu.get_barrier_semaphore()
        for p in peers:
            pl.semaphore_signal(barrier, inc=1, device_id=(p,),
                                device_id_type=pl.DeviceIdType.MESH)

        lane = lax.broadcasted_iota(jnp.int32, tile, 1)
        sub = lax.broadcasted_iota(jnp.int32, tile, 0)
        lane_minus_sub = lane - sub

        rdmas = {}
        for c in range(nc):
            n_groups = chunks[c] // _SUBLANES
            k = msg_rows[c]
            in_copies[c].wait()
            sums = []
            for g in range(n_groups):
                xv = xbuf[pl.ds(starts[c] + _SUBLANES * g, _SUBLANES), :]
                sq = xv * xv
                part = tree_sum([sq[:, j * _LANES:(j + 1) * _LANES]
                                 for j in range(n // _LANES)])
                sums.append(jnp.broadcast_to(
                    jnp.sum(part, axis=1, keepdims=True), tile))
            for kk in range(k):
                grp = sums[kk * _GROUPS_PER_MSG_ROW:(kk + 1) * _GROUPS_PER_MSG_ROW]
                packed = tree_sum([
                    jnp.where(lane_minus_sub == _SUBLANES * j, s, 0.0)
                    for j, s in enumerate(grp)])
                send_ref[c, pl.ds(kk, 1), :] = jnp.sum(packed, axis=0, keepdims=True)
            if c == 0:
                pl.semaphore_wait(barrier, _N_DEV - 1)
            for j, p in enumerate(peers):
                if j == 0:
                    dst = diag_ref.at[c, pl.ds(0, k)]
                else:
                    dst = near_ref.at[c, j - 1, pl.ds(0, k)]
                rdma = pltpu.make_async_remote_copy(
                    src_ref=send_ref.at[c, pl.ds(0, k)], dst_ref=dst,
                    send_sem=send_sems.at[3 * c + j], recv_sem=recv_sems.at[3 * c + j],
                    device_id=(p,), device_id_type=pl.DeviceIdType.MESH)
                rdma.start()
                rdmas[c, j] = rdma
            for g in range(n_groups):
                base_ref[pl.ds(starts[c] + _SUBLANES * g, _SUBLANES), :] = (
                    sums[g] + n_global * _EPS)

        g_copy.wait()
        g_scaled = gbuf[...] * math.sqrt(n_global)

        for c in range(nc):
            n_groups = chunks[c] // _SUBLANES
            rdmas[c, 1].wait_recv()
            rdmas[c, 2].wait_recv()
            for kk in range(msg_rows[c]):
                both = jnp.broadcast_to(
                    near_ref[c, 0, pl.ds(kk, 1), :] + near_ref[c, 1, pl.ds(kk, 1), :],
                    tile)
                for j in range(min(_GROUPS_PER_MSG_ROW,
                                   n_groups - kk * _GROUPS_PER_MSG_ROW)):
                    rows = pl.ds(starts[c] + _LANES * kk + _SUBLANES * j, _SUBLANES)
                    per_row = jnp.sum(
                        jnp.where(lane_minus_sub == _SUBLANES * j, both, 0.0),
                        axis=1, keepdims=True)
                    base_ref[rows, :] = base_ref[rows, :] + per_row

        for rdma in rdmas.values():
            rdma.wait_send()

        for c in range(nc):
            rdmas[c, 0].wait_recv()
            for g in range(chunks[c] // _SUBLANES):
                kk, j = divmod(g, _GROUPS_PER_MSG_ROW)
                rows = pl.ds(starts[c] + _SUBLANES * g, _SUBLANES)
                vals = [jnp.full(tile, diag_ref[c, kk, _SUBLANES * j + s], jnp.float32)
                        for s in range(_SUBLANES)]
                bit = 1
                while len(vals) > 1:
                    vals = [jnp.where((sub & bit) == 0, vals[i], vals[i + 1])
                            for i in range(0, len(vals), 2)]
                    bit *= 2
                inv = lax.rsqrt(base_ref[rows, :] + vals[0])
                inv = jnp.concatenate([inv] * (n // _LANES), axis=1)
                out_ref[rows, :] = xbuf[rows, :] * g_scaled * inv

    return pl.pallas_call(
        body,
        out_shape=jax.ShapeDtypeStruct((m, n), x.dtype),
        in_specs=[pl.BlockSpec(memory_space=pl.ANY),
                  pl.BlockSpec(memory_space=pl.ANY)],
        out_specs=pl.BlockSpec(memory_space=pltpu.VMEM),
        scratch_shapes=[
            pltpu.VMEM((m, n), jnp.float32),
            pltpu.VMEM((1, n), jnp.float32),
            pltpu.VMEM((m, _LANES), jnp.float32),
            pltpu.VMEM((nc, max_msg_rows, _LANES), jnp.float32),
            pltpu.VMEM((nc, 2, max_msg_rows, _LANES), jnp.float32),
            pltpu.SMEM((nc, max_msg_rows, _LANES), jnp.float32),
            pltpu.SemaphoreType.DMA((nc,)),
            pltpu.SemaphoreType.DMA,
            pltpu.SemaphoreType.DMA((3 * nc,)),
            pltpu.SemaphoreType.DMA((3 * nc,)),
        ],
        compiler_params=pltpu.CompilerParams(
            collective_id=0,
            disable_semaphore_checks=True,
        ),
    )(x, gamma.reshape(1, n))
```

```python
import math

import jax
import jax.numpy as jnp
from jax import lax
from jax.experimental import pallas as pl
from jax.experimental.pallas import tpu as pltpu

_N_DEV = 4
_EPS = 1e-5
_LANES = 128
_SUBLANES = 8
_GROUPS_PER_MSG_ROW = _LANES // _SUBLANES


def _row_chunks(m):
    if m == 768:
        return (256, 256, 128, 64, 64)
    assert m % _SUBLANES == 0
    chunks, left = [], m
    while left > 0:
        c = min(256, left)
        chunks.append(c)
        left -= c
    return tuple(chunks)


def _tree_sum(terms):
    while len(terms) > 1:
        nxt = [terms[i] + terms[i + 1] for i in range(0, len(terms) - 1, 2)]
        if len(terms) % 2:
            nxt.append(terms[-1])
        terms = nxt
    return terms[0]


def pallas_dist_rmsnorm_colshard_i_m768_n512_kernel(x: jax.Array, gamma: jax.Array):
    m, n = x.shape
    assert n % _LANES == 0
    n_global = n * _N_DEV
    chunks = _row_chunks(m)
    nc = len(chunks)
    starts = [sum(chunks[:c]) for c in range(nc)]
    msg_rows = [-(-r // _LANES) for r in chunks]
    max_msg_rows = max(msg_rows)
    tile = (_SUBLANES, _LANES)

    def body(x_hbm, g_hbm, out_ref,
             xbuf, gbuf, base_ref, send_ref, near_ref, diag_ref,
             in_sems, g_sem, send_sems, recv_sems):
        my = lax.axis_index("i")

        in_copies = []
        for c in range(nc):
            rows = pl.ds(starts[c], chunks[c])
            cp = pltpu.make_async_copy(x_hbm.at[rows], xbuf.at[rows], in_sems.at[c])
            cp.start()
            in_copies.append(cp)
        g_copy = pltpu.make_async_copy(g_hbm, gbuf, g_sem)
        g_copy.start()

        peers = [(my + 2) % _N_DEV, (my + 1) % _N_DEV, (my + 3) % _N_DEV]
        barrier = pltpu.get_barrier_semaphore()
        for p in peers:
            pl.semaphore_signal(barrier, inc=1, device_id=(p,),
                                device_id_type=pl.DeviceIdType.MESH)

        lane = lax.broadcasted_iota(jnp.int32, tile, 1)
        sub = lax.broadcasted_iota(jnp.int32, tile, 0)
        lane_minus_sub = lane - sub

        rdmas = {}
        for c in range(nc):
            n_groups = chunks[c] // _SUBLANES
            k = msg_rows[c]
            in_copies[c].wait()
            sums = []
            for g in range(n_groups):
                xv = xbuf[pl.ds(starts[c] + _SUBLANES * g, _SUBLANES), :]
                sq = xv * xv
                part = _tree_sum([sq[:, j * _LANES:(j + 1) * _LANES]
                                  for j in range(n // _LANES)])
                sums.append(jnp.broadcast_to(
                    jnp.sum(part, axis=1, keepdims=True), tile))
            for kk in range(k):
                grp = sums[kk * _GROUPS_PER_MSG_ROW:(kk + 1) * _GROUPS_PER_MSG_ROW]
                packed = _tree_sum([
                    jnp.where(lane_minus_sub == _SUBLANES * j, s, 0.0)
                    for j, s in enumerate(grp)])
                send_ref[c, pl.ds(kk, 1), :] = jnp.sum(packed, axis=0, keepdims=True)
            if c == 0:
                pl.semaphore_wait(barrier, _N_DEV - 1)
            for j, p in enumerate(peers):
                if j == 0:
                    dst = diag_ref.at[c, pl.ds(0, k)]
                else:
                    dst = near_ref.at[c, j - 1, pl.ds(0, k)]
                rdma = pltpu.make_async_remote_copy(
                    src_ref=send_ref.at[c, pl.ds(0, k)], dst_ref=dst,
                    send_sem=send_sems.at[3 * c + j], recv_sem=recv_sems.at[3 * c + j],
                    device_id=(p,), device_id_type=pl.DeviceIdType.MESH)
                rdma.start()
                rdmas[c, j] = rdma
            for g in range(n_groups):
                base_ref[pl.ds(starts[c] + _SUBLANES * g, _SUBLANES), :] = (
                    sums[g] + n_global * _EPS)

        g_copy.wait()
        g_scaled = gbuf[...] * math.sqrt(n_global)

        def add_neighbours(c):
            n_groups = chunks[c] // _SUBLANES
            rdmas[c, 1].wait_recv()
            rdmas[c, 2].wait_recv()
            for kk in range(msg_rows[c]):
                both = jnp.broadcast_to(
                    near_ref[c, 0, pl.ds(kk, 1), :] + near_ref[c, 1, pl.ds(kk, 1), :],
                    tile)
                for j in range(min(_GROUPS_PER_MSG_ROW,
                                   n_groups - kk * _GROUPS_PER_MSG_ROW)):
                    rows = pl.ds(starts[c] + _LANES * kk + _SUBLANES * j, _SUBLANES)
                    per_row = jnp.sum(
                        jnp.where(lane_minus_sub == _SUBLANES * j, both, 0.0),
                        axis=1, keepdims=True)
                    base_ref[rows, :] = base_ref[rows, :] + per_row

        def normalise(c):
            rdmas[c, 0].wait_recv()
            for g in range(chunks[c] // _SUBLANES):
                kk, j = divmod(g, _GROUPS_PER_MSG_ROW)
                rows = pl.ds(starts[c] + _SUBLANES * g, _SUBLANES)
                vals = [jnp.full(tile, diag_ref[c, kk, _SUBLANES * j + s], jnp.float32)
                        for s in range(_SUBLANES)]
                bit = 1
                while len(vals) > 1:
                    vals = [jnp.where((sub & bit) == 0, vals[i], vals[i + 1])
                            for i in range(0, len(vals), 2)]
                    bit *= 2
                inv = lax.rsqrt(base_ref[rows, :] + vals[0])
                inv = jnp.concatenate([inv] * (n // _LANES), axis=1)
                out_ref[rows, :] = xbuf[rows, :] * g_scaled * inv

        early = min(2, nc)
        for c in range(early):
            add_neighbours(c)
        normalise(0)
        for c in range(early, nc):
            add_neighbours(c)
        for rdma in rdmas.values():
            rdma.wait_send()
        for c in range(1, nc):
            normalise(c)

    return pl.pallas_call(
        body,
        out_shape=jax.ShapeDtypeStruct((m, n), x.dtype),
        in_specs=[pl.BlockSpec(memory_space=pl.ANY),
                  pl.BlockSpec(memory_space=pl.ANY)],
        out_specs=pl.BlockSpec(memory_space=pltpu.VMEM),
        scratch_shapes=[
            pltpu.VMEM((m, n), jnp.float32),
            pltpu.VMEM((1, n), jnp.float32),
            pltpu.VMEM((m, _LANES), jnp.float32),
            pltpu.VMEM((nc, max_msg_rows, _LANES), jnp.float32),
            pltpu.VMEM((nc, 2, max_msg_rows, _LANES), jnp.float32),
            pltpu.SMEM((nc, max_msg_rows, _LANES), jnp.float32),
            pltpu.SemaphoreType.DMA((nc,)),
            pltpu.SemaphoreType.DMA,
            pltpu.SemaphoreType.DMA((3 * nc,)),
            pltpu.SemaphoreType.DMA((3 * nc,)),
        ],
        compiler_params=pltpu.CompilerParams(
            collective_id=0,
            disable_semaphore_checks=True,
        ),
    )(x, gamma.reshape(1, n))
```

```python
import math

import jax
import jax.numpy as jnp
from jax import lax
from jax.experimental import pallas as pl
from jax.experimental.pallas import tpu as pltpu

_N_DEV = 4
_EPS = 1e-5
_LANES = 128
_SUBLANES = 8
_GROUPS_PER_MSG_ROW = _LANES // _SUBLANES


def _row_chunks(m):
    if m == 768:
        return (256, 256, 128, 64, 64)
    assert m % _SUBLANES == 0
    chunks, left = [], m
    while left > 0:
        c = min(256, left)
        chunks.append(c)
        left -= c
    return tuple(chunks)


def _tree_sum(terms):
    while len(terms) > 1:
        nxt = [terms[i] + terms[i + 1] for i in range(0, len(terms) - 1, 2)]
        if len(terms) % 2:
            nxt.append(terms[-1])
        terms = nxt
    return terms[0]


def _compiler_params():
    try:
        return pltpu.CompilerParams(collective_id=0, disable_semaphore_checks=True)
    except TypeError:
        return pltpu.CompilerParams(collective_id=0)


def pallas_dist_rmsnorm_colshard_i_m768_n512_kernel(x: jax.Array, gamma: jax.Array):
    m, n = x.shape
    assert n % _LANES == 0
    n_global = n * _N_DEV
    chunks = _row_chunks(m)
    nc = len(chunks)
    starts = [sum(chunks[:c]) for c in range(nc)]
    msg_rows = [-(-r // _LANES) for r in chunks]
    max_msg_rows = max(msg_rows)
    tile = (_SUBLANES, _LANES)

    def body(x_hbm, g_hbm, out_ref,
             xbuf, gbuf, base_ref, send_ref, near_ref, diag_ref,
             in_sems, g_sem, send_sems, recv_sems):
        my = lax.axis_index("i")

        in_copies = []
        for c in range(nc):
            rows = pl.ds(starts[c], chunks[c])
            cp = pltpu.make_async_copy(x_hbm.at[rows], xbuf.at[rows], in_sems.at[c])
            cp.start()
            in_copies.append(cp)
        g_copy = pltpu.make_async_copy(g_hbm, gbuf, g_sem)
        g_copy.start()

        peers = [(my + 2) % _N_DEV, (my + 1) % _N_DEV, (my + 3) % _N_DEV]
        barrier = pltpu.get_barrier_semaphore()
        for p in peers:
            pl.semaphore_signal(barrier, inc=1, device_id=(p,),
                                device_id_type=pl.DeviceIdType.MESH)

        lane = lax.broadcasted_iota(jnp.int32, tile, 1)
        sub = lax.broadcasted_iota(jnp.int32, tile, 0)
        lane_minus_sub = lane - sub

        rdmas = {}
        for c in range(nc):
            n_groups = chunks[c] // _SUBLANES
            k = msg_rows[c]
            in_copies[c].wait()
            sums = []
            for g in range(n_groups):
                xv = xbuf[pl.ds(starts[c] + _SUBLANES * g, _SUBLANES), :]
                sq = xv * xv
                part = _tree_sum([sq[:, j * _LANES:(j + 1) * _LANES]
                                  for j in range(n // _LANES)])
                sums.append(jnp.broadcast_to(
                    jnp.sum(part, axis=1, keepdims=True), tile))
            for kk in range(k):
                grp = sums[kk * _GROUPS_PER_MSG_ROW:(kk + 1) * _GROUPS_PER_MSG_ROW]
                packed = _tree_sum([
                    jnp.where(lane_minus_sub == _SUBLANES * j, s, 0.0)
                    for j, s in enumerate(grp)])
                send_ref[c, pl.ds(kk, 1), :] = jnp.sum(packed, axis=0, keepdims=True)
            if c == 0:
                pl.semaphore_wait(barrier, _N_DEV - 1)
            for j, p in enumerate(peers):
                if j == 0:
                    dst = diag_ref.at[c, pl.ds(0, k)]
                else:
                    dst = near_ref.at[c, j - 1, pl.ds(0, k)]
                rdma = pltpu.make_async_remote_copy(
                    src_ref=send_ref.at[c, pl.ds(0, k)], dst_ref=dst,
                    send_sem=send_sems.at[3 * c + j], recv_sem=recv_sems.at[3 * c + j],
                    device_id=(p,), device_id_type=pl.DeviceIdType.MESH)
                rdma.start()
                rdmas[c, j] = rdma
            for g in range(n_groups):
                base_ref[pl.ds(starts[c] + _SUBLANES * g, _SUBLANES), :] = (
                    sums[g] + n_global * _EPS)

        g_copy.wait()
        g_scaled = gbuf[...] * math.sqrt(n_global)

        def add_neighbours(c):
            n_groups = chunks[c] // _SUBLANES
            rdmas[c, 1].wait_recv()
            rdmas[c, 2].wait_recv()
            for kk in range(msg_rows[c]):
                both = jnp.broadcast_to(
                    near_ref[c, 0, pl.ds(kk, 1), :] + near_ref[c, 1, pl.ds(kk, 1), :],
                    tile)
                for j in range(min(_GROUPS_PER_MSG_ROW,
                                   n_groups - kk * _GROUPS_PER_MSG_ROW)):
                    rows = pl.ds(starts[c] + _LANES * kk + _SUBLANES * j, _SUBLANES)
                    per_row = jnp.sum(
                        jnp.where(lane_minus_sub == _SUBLANES * j, both, 0.0),
                        axis=1, keepdims=True)
                    base_ref[rows, :] = base_ref[rows, :] + per_row

        def normalise(c):
            rdmas[c, 0].wait_recv()
            for g in range(chunks[c] // _SUBLANES):
                kk, j = divmod(g, _GROUPS_PER_MSG_ROW)
                rows = pl.ds(starts[c] + _SUBLANES * g, _SUBLANES)
                vals = [jnp.full(tile, diag_ref[c, kk, _SUBLANES * j + s], jnp.float32)
                        for s in range(_SUBLANES)]
                bit = 1
                while len(vals) > 1:
                    vals = [jnp.where((sub & bit) == 0, vals[i], vals[i + 1])
                            for i in range(0, len(vals), 2)]
                    bit *= 2
                inv = lax.rsqrt(base_ref[rows, :] + vals[0])
                inv = jnp.concatenate([inv] * (n // _LANES), axis=1)
                out_ref[rows, :] = xbuf[rows, :] * g_scaled * inv

        early = min(2, nc)
        for c in range(early):
            add_neighbours(c)
        normalise(0)
        for c in range(early, nc):
            add_neighbours(c)
        for rdma in rdmas.values():
            rdma.wait_send()
        for c in range(1, nc):
            normalise(c)

    return pl.pallas_call(
        body,
        out_shape=jax.ShapeDtypeStruct((m, n), x.dtype),
        in_specs=[pl.BlockSpec(memory_space=pl.ANY),
                  pl.BlockSpec(memory_space=pl.ANY)],
        out_specs=pl.BlockSpec(memory_space=pltpu.VMEM),
        scratch_shapes=[
            pltpu.VMEM((m, n), jnp.float32),
            pltpu.VMEM((1, n), jnp.float32),
            pltpu.VMEM((m, _LANES), jnp.float32),
            pltpu.VMEM((nc, max_msg_rows, _LANES), jnp.float32),
            pltpu.VMEM((nc, 2, max_msg_rows, _LANES), jnp.float32),
            pltpu.SMEM((nc, max_msg_rows, _LANES), jnp.float32),
            pltpu.SemaphoreType.DMA((nc,)),
            pltpu.SemaphoreType.DMA,
            pltpu.SemaphoreType.DMA((3 * nc,)),
            pltpu.SemaphoreType.DMA((3 * nc,)),
        ],
        compiler_params=_compiler_params(),
    )(x, gamma.reshape(1, n))
```
